```python
import numpy as np

kernel_name = "dist_layernorm_xy_m512_n256"

def setup_inputs():
    x = np.random.randn(1024, 512).astype(np.float32)
    gamma = np.random.randn(512).astype(np.float32)
    beta = np.random.randn(512).astype(np.float32)
    return {"x": x, "gamma": gamma, "beta": beta}

def reference(x: np.ndarray, gamma: np.ndarray, beta: np.ndarray) -> np.ndarray:
    eps = 1e-5
    mean = np.mean(x, axis=1, keepdims=True)
    var = np.var(x, axis=1, keepdims=True)
    return gamma * (x - mean) / np.sqrt(var + eps) + beta
```

```python
import math

import jax
import jax.numpy as jnp
from jax import lax
from jax.experimental import pallas as pl
from jax.experimental.pallas import tpu as pltpu

EPS = 1e-5
SUBLANES, LANES = 8, 128

CHUNK_ROWS = (16,) + (48,) * 10
RAW_ROWS = 16
DEFERRED_GROUPS = 5

MAX_MEAN_SQ_OVER_VAR = 6.0
UNSAFE_WORD = 0x7B000000
SIGN_BIT = -0x80000000
HIGH_HALF = -0x10000
HALF_ULP = 0x8000


def _as_int(v):
    return lax.bitcast_convert_type(v, jnp.int32)


def _as_float(v):
    return lax.bitcast_convert_type(v, jnp.float32)


def _row_sum(v):
    return jnp.sum(v, axis=1, keepdims=True)


def _inv_sqrt(v):
    return jnp.exp2(jnp.log2(v) * -0.5)


def _pack_words(u, s2, n_total):
    uu = u * u
    t = (s2 + n_total * EPS / 2) - uu
    margin = s2 * (0.5 / (1 + 1 / MAX_MEAN_SQ_OVER_VAR)) - uu
    low = lax.shift_right_logical(_as_int(u) + HALF_ULP, 16)
    high = (_as_int(t) + (HALF_ULP - low)) & HIGH_HALF
    return high | (low | (_as_int(margin) & SIGN_BIT))


def _kernel(
    x_hbm, gamma_hbm, beta_hbm, out_ref,
    x_ref, gamma_ref, beta_ref, terms_ref, y_ref,
    words_out, words_in, raw_in, exact_out, exact_in,
    chunk_sems, load_sems, words_send_sems, words_recv_sems, raw_sems, exact_sems,
):
    m, n = x_ref.shape
    n_total = 2 * n
    root_n = math.sqrt(n_total)
    n_chunks = len(CHUNK_ROWS)
    starts = [sum(CHUNK_ROWS[:i]) for i in range(n_chunks)]
    raw_start = m - RAW_ROWS
    halves = [slice(h * LANES, (h + 1) * LANES) for h in range(n // LANES)]
    tile = (SUBLANES, LANES)

    def groups(i):
        return range(starts[i], starts[i] + CHUNK_ROWS[i], SUBLANES)

    def rows(r):
        return slice(r, r + SUBLANES)

    my_x, my_y = lax.axis_index("x"), lax.axis_index("y")

    def to_peer(src, dst, send_sem, recv_sem):
        return pltpu.make_async_remote_copy(
            src, dst, send_sem, recv_sem,
            device_id=(my_x, 1 - my_y), device_id_type=pl.DeviceIdType.MESH,
        )

    chunk_loads = []
    for i, size in enumerate(CHUNK_ROWS):
        span = pl.ds(starts[i], size)
        chunk_loads.append(
            pltpu.make_async_copy(x_hbm.at[span], x_ref.at[span], chunk_sems.at[i])
        )
        chunk_loads[i].start()

    raw_span = pl.ds(raw_start, RAW_ROWS)
    raw_copy = to_peer(x_hbm.at[raw_span], raw_in, raw_sems.at[0], raw_sems.at[1])
    packets = [
        to_peer(
            words_out.at[i], words_in.at[i], words_send_sems.at[i], words_recv_sems.at[i]
        )
        for i in range(n_chunks)
    ]

    barrier = pltpu.get_barrier_semaphore()
    pl.semaphore_signal(
        barrier, inc=1,
        device_id=(my_x, 1 - my_y), device_id_type=pl.DeviceIdType.MESH,
    )

    streams = my_y == 1

    @pl.when(streams)
    def _():
        pl.semaphore_wait(barrier, 1)
        raw_copy.start()

    other_loads = [
        pltpu.make_async_copy(gamma_hbm, gamma_ref, load_sems.at[0]),
        pltpu.make_async_copy(beta_hbm, beta_ref, load_sems.at[1]),
        pltpu.make_async_copy(x_hbm.at[raw_span], x_ref.at[raw_span], load_sems.at[2]),
    ]
    for load in other_loads:
        load.start()

    lane = lax.broadcasted_iota(jnp.int32, tile, 1)
    sublane = lax.broadcasted_iota(jnp.int32, tile, 0)
    spare_lane = lane[0:1] == LANES - 1
    sums = {}

    def send_packet(i, ordering_value=None):
        u = s2 = jnp.zeros(tile, jnp.float32)
        for r in groups(i):
            here = lane - sublane == r - starts[i]
            u = jnp.where(here, sums[r][0], u)
            s2 = jnp.where(here, sums[r][1], s2)
        words = _pack_words(u, s2, n_total)
        words = jnp.take_along_axis(words, lane & (SUBLANES - 1), axis=0)[0:1]
        if ordering_value is not None:
            words = jnp.where(spare_lane, _as_int(ordering_value)[0:1], words)
        words_out[i] = words
        pl.when(streams)(packets[i].start)

    for i in range(n_chunks):
        chunk_loads[i].wait()
        partials = None
        for r in groups(i):
            a, b = (x_ref[rows(r), cols] for cols in halves)
            p1, p2 = (a + b) * (1 / root_n), a * a + b * b
            sums[r] = (_row_sum(p1), _row_sum(p2))
            partials = p1 + p2 if partials is None else (partials + p1) + p2
        if i > 0:
            send_packet(i - 1, partials if i < n_chunks - 1 else None)
    send_packet(n_chunks - 1)

    for load in other_loads:
        load.wait()
    gamma_rows = [gamma_ref[cols].reshape(1, LANES) for cols in halves]
    beta_rows = [beta_ref[cols].reshape(1, LANES) for cols in halves]
    gamma = [jnp.broadcast_to(v, tile) for v in gamma_rows]
    beta = [jnp.broadcast_to(v, tile) for v in beta_rows]

    zero = pl.multiple_of((my_x >> 1) * SUBLANES, SUBLANES)

    def stored(r):
        return pl.ds(zero + r, SUBLANES)

    unsafe = jnp.zeros((1, LANES), jnp.float32)
    for i in range(n_chunks):
        words = words_out[i]
        unsafe = jnp.where((words < 0) | (words >= UNSAFE_WORD), 1.0, unsafe)
    sent_unsafe = jnp.max(jnp.where(spare_lane, 0.0, unsafe)) > 0

    for r in range(0, raw_start, SUBLANES):
        a, b = (x_ref[stored(r), cols] for cols in halves)
        u = jnp.broadcast_to(_row_sum((a + b) * (1 / root_n)), tile)
        s2 = _row_sum(a * a + b * b)
        terms_ref[0, rows(r), :] = u + u
        terms_ref[1, rows(r), :] = (s2 + n_total * EPS / 2) - u * u
        y_ref[0, rows(r), :] = (a * root_n - u) * gamma[0]
        y_ref[1, rows(r), :] = (b * root_n - u) * gamma[1]
    for r in range(raw_start, m, SUBLANES):
        a, b = (x_ref[rows(r), cols] for cols in halves)
        half_row_mean = jnp.broadcast_to(_row_sum(a + b) * (1 / n), tile)
        terms_ref[0, rows(r), :] = half_row_mean
        y_ref[0, rows(r), :] = a - half_row_mean
        y_ref[1, rows(r), :] = b - half_row_mean

    @pl.when(jnp.logical_not(streams))
    def _():
        pl.semaphore_wait(barrier, 1)
        for packet in packets:
            packet.start()
        raw_copy.start()

    for packet in packets:
        packet.wait_send()
    raw_copy.wait_send()

    def store(span, results):
        out_ref[span, :] = jnp.concatenate(results, axis=1).astype(out_ref.dtype)

    raw_copy.wait_recv()
    for r in range(raw_start, m, SUBLANES):
        d = [y_ref[h, stored(r), :] for h in range(2)]
        d += [
            raw_in[rows(r - raw_start), cols] - terms_ref[0, stored(r), :]
            for cols in halves
        ]
        s1 = _row_sum((d[0] + d[1]) + (d[2] + d[3]))
        s2 = _row_sum((d[0] * d[0] + d[1] * d[1]) + (d[2] * d[2] + d[3] * d[3]))
        shift = jnp.broadcast_to(s1, tile) * (1 / n_total)
        rstd = _inv_sqrt((s2 - shift * s1) * (1 / n_total) + EPS)
        store(rows(r), [(d[h] - shift) * gamma[h] * rstd + beta[h] for h in range(2)])

    largest_word = jnp.uint32(0)
    deferred = []
    for i in range(n_chunks):
        packets[i].wait_recv()
        arrived = []
        for r in groups(i):
            scalars = [words_in[i, 0, r - starts[i] + s] for s in range(SUBLANES)]
            for word in scalars:
                unsigned = lax.bitcast_convert_type(word, jnp.uint32)
                largest_word = jnp.maximum(largest_word, unsigned)
            splats = [jnp.full(tile, word, jnp.int32) for word in scalars]
            words = splats[0]
            for s in range(1, SUBLANES):
                words = jnp.where(sublane == s, splats[s], words)
            arrived.append((r, words))
        keep = min(DEFERRED_GROUPS, len(arrived)) if i < n_chunks - 1 else 0
        for r, words in deferred + arrived[: len(arrived) - keep]:
            u = _as_float(words << 16)
            scale = _inv_sqrt(
                (_as_float(words) + terms_ref[1, stored(r), :])
                - u * terms_ref[0, stored(r), :]
            )
            store(
                rows(r),
                [(y_ref[h, stored(r), :] - u * gamma[h]) * scale + beta[h] for h in range(2)],
            )
        deferred = arrived[len(arrived) - keep :]

    @pl.when(sent_unsafe | (largest_word >= jnp.uint32(UNSAFE_WORD)))
    def _():
        square = (LANES, LANES)

        def block(j):
            return pl.ds(pl.multiple_of(j * LANES, LANES), LANES)

        @pl.loop(0, m // LANES)
        def _(j):
            x = x_ref[block(j), :]
            mean = _row_sum(x) * (1 / n)
            centered = x - mean
            m2 = _row_sum(centered * centered)
            exact_out[2 * j] = jnp.broadcast_to(mean, square).T[0:1]
            exact_out[2 * j + 1] = jnp.broadcast_to(m2, square).T[0:1]

        exact_copy = to_peer(exact_out, exact_in, exact_sems.at[0], exact_sems.at[1])
        exact_copy.start()
        exact_copy.wait()

        @pl.loop(0, m // LANES)
        def _(j):
            mean_a, mean_b = exact_out[2 * j], exact_in[2 * j]
            m2 = exact_out[2 * j + 1] + exact_in[2 * j + 1]
            var = m2 * (1 / n_total) + jnp.square((mean_a - mean_b) * 0.5)
            mean = jnp.broadcast_to(0.5 * mean_a + 0.5 * mean_b, square).T
            rstd = jnp.broadcast_to(lax.rsqrt(var + EPS), square).T
            store(
                block(j),
                [
                    (x_ref[block(j), cols] - mean) * rstd * gamma_rows[h] + beta_rows[h]
                    for h, cols in enumerate(halves)
                ],
            )


def pallas_dist_layernorm_xy_m512_n256_kernel(
    x: jax.Array,
    gamma: jax.Array,
    beta: jax.Array,
):
    m, n = x.shape
    assert (m, n) == (sum(CHUNK_ROWS) + RAW_ROWS, 2 * LANES)
    n_chunks = len(CHUNK_ROWS)
    f32, dma = jnp.float32, pltpu.SemaphoreType.DMA
    return pl.pallas_call(
        _kernel,
        out_shape=jax.ShapeDtypeStruct((m, n), jnp.bfloat16),
        in_specs=[pl.BlockSpec(memory_space=pltpu.HBM)] * 3,
        out_specs=pl.BlockSpec(memory_space=pltpu.VMEM),
        scratch_shapes=[
            pltpu.VMEM((m, n), f32),
            pltpu.VMEM((n,), f32),
            pltpu.VMEM((n,), f32),
            pltpu.VMEM((2, m, LANES), f32),
            pltpu.VMEM((2, m, LANES), f32),
            pltpu.VMEM((n_chunks, 1, LANES), jnp.int32),
            pltpu.SMEM((n_chunks, 1, LANES), jnp.int32),
            pltpu.VMEM((RAW_ROWS, n), f32),
            pltpu.VMEM((2 * m // LANES, 1, LANES), f32),
            pltpu.VMEM((2 * m // LANES, 1, LANES), f32),
            dma((n_chunks,)),
            dma((3,)),
            dma((n_chunks,)),
            dma((n_chunks,)),
            dma((2,)),
            dma((2,)),
        ],
        compiler_params=pltpu.CompilerParams(
            collective_id=0,
            disable_bounds_checks=True,
            disable_semaphore_checks=True,
            flags={"XLA_TPU_RESCHEDULE_DMA_DONES": True},
        ),
    )(x, gamma, beta)
```
